```python
import numpy as np

kernel_name = "dist_moe_cap_ep_outshard_n2048_d512_e8_h1024"

def setup_inputs():
    x = np.random.randn(2048, 512).astype(np.float32)
    router_W = np.random.randn(512, 32).astype(np.float32) * 0.1
    scores64 = x.astype(np.float64) @ router_W.astype(np.float64)
    route_idx = np.argsort(-scores64, axis=-1)[:, :1].astype(np.int32)
    expert_W = np.random.randn(32, 512, 1024).astype(np.float32) * 0.02
    return {"x": x, "router_W": router_W, "route_idx": route_idx, "expert_W": expert_W}

def reference(x, router_W, route_idx, expert_W):
    counts = np.zeros(32, dtype=np.int64)
    out = np.zeros((2048, 1024), dtype=np.float32)
    for i in range(2048):
        e = int(route_idx[i, 0])
        if counts[e] < 51:
            out[i] = x[i] @ expert_W[e]
            counts[e] += 1
    return out
```

```python
import jax
import jax.numpy as jnp
from jax import lax
from jax.experimental import pallas as pl
from jax.experimental.pallas import tpu as pltpu

N_DEV = 4
N_TOK = 2048
D = 512
H = 1024
N_EXP = 32
E_LOC = N_EXP // N_DEV
CAP = 51
SLOTS = 64
T_LOC = N_TOK // N_DEV
ROWS = N_TOK // 128
NG = H // 256
PHASES = ((0, 3), (3, 1))
W_AHEAD = 2

f32, bf16, i32, u32 = jnp.float32, jnp.bfloat16, jnp.int32, jnp.uint32


def _iota(shape, dim):
    return lax.broadcasted_iota(i32, shape, dim)


def _mm(a, b):
    return jnp.dot(a, b, preferred_element_type=f32)


def _mm_nt(a, b):
    return lax.dot_general(a, b, (((1,), (1,)), ((), ())), preferred_element_type=f32)


def _onehot(cond):
    return jnp.where(cond, 1.0, 0.0).astype(bf16)


def _pack(lo, hi):
    lo = lax.bitcast_convert_type(lo.astype(bf16).astype(f32), u32)
    hi = lax.bitcast_convert_type(hi.astype(bf16).astype(f32), u32)
    return (lo >> 16) | (hi & jnp.uint32(0xFFFF0000))


def _unpack(u):
    lo = lax.bitcast_convert_type(u << 16, f32).astype(bf16)
    hi = lax.bitcast_convert_type(u & jnp.uint32(0xFFFF0000), f32).astype(bf16)
    return lo, hi


def _body(x_hbm, idx_hbm, w_hbm, out_hbm,
          idx_v, row_v, tab_v, tab_s, xg, xb, wbuf, ybuf, rbuf, pmat, obuf,
          misc_sem, w_sem, g_sem, send_sem, recv_sem, out_sem, done_sem):
    me = lax.axis_index("i")

    steps = [(e, g0, ng) for (g0, ng) in PHASES for e in range(E_LOC)]

    def w_copy(i):
        e, g0, ng = steps[i]
        cols = pl.ds(g0 * 256, ng * 256)
        return pltpu.make_async_copy(w_hbm.at[e, :, cols], wbuf.at[e, :, cols], w_sem.at[i])

    idx_cp = pltpu.make_async_copy(idx_hbm, idx_v, misc_sem.at[0])
    idx_cp.start()
    for i in range(W_AHEAD):
        w_copy(i).start()

    barrier = pltpu.get_barrier_semaphore()
    for k in range(1, N_DEV):
        pl.semaphore_signal(barrier, inc=1, device_id=((me + k) % N_DEV,),
                            device_id_type=pl.DeviceIdType.MESH)

    xg[:, 48:SLOTS, :] = jnp.zeros((E_LOC, SLOTS - 48, D), f32)

    li = _iota((128, 128), 1)
    si = _iota((128, 128), 0)
    u_strict = _onehot(si < li)
    ones = jnp.ones((128, 128), bf16)
    n_er = N_EXP * ROWS
    rr = _iota((n_er, n_er), 0)
    cc = _iota((n_er, n_er), 1)
    l_blk = _onehot(((rr >> 4) == (cc >> 4)) & (cc < rr))

    idx_cp.wait()
    idx = idx_v[...] & (N_EXP - 1)

    er = _iota((n_er, 128), 0)
    m = jnp.concatenate([idx] * N_EXP, axis=0) == (er >> 4)
    mb = _onehot(m)
    within = _mm(mb, u_strict)
    tot = _mm(mb, ones)
    before = _mm(l_blk, tot.astype(bf16))
    pe = jnp.where(m, within + before, 0.0)
    pos = pe[0:ROWS]
    for e in range(1, N_EXP):
        pos = pos + pe[e * ROWS:(e + 1) * ROWS]
    pos = pos.astype(i32)
    ok = pos < CAP
    row_v[0:ROWS, :] = idx
    row_v[ROWS:2 * ROWS, :] = jnp.where(ok, 1, 0)

    key = jnp.where(ok & ((idx >> 3) == me), (idx & 7) * SLOTS + pos, -1)
    slot_i = _iota((E_LOC * SLOTS, 128), 0)
    acc = jnp.zeros((E_LOC * SLOTS, 128), i32)
    for r in range(ROWS):
        acc = jnp.where(slot_i == key[r:r + 1, :], r + 1, acc)
    s8 = _iota((8, 128), 0)
    l8 = _iota((8, 128), 1)
    hi = _mm_nt(jnp.ones((8, 128), bf16), acc.astype(f32).astype(bf16))
    lo = _mm_nt(l8.astype(f32).astype(bf16), _onehot(acc > 0))
    tok = jnp.maximum((hi.astype(i32) - 1) * 128 + lo.astype(i32), 0)
    for j in range(4):
        tab_v[24 + j:25 + j, :] = tok[0:1, j * 128:(j + 1) * 128]

    diag = _iota((n_er, 128), 1) == (er >> 4)
    z0 = jnp.where(diag, jnp.minimum(before, CAP), 0.0).astype(bf16)
    z1 = jnp.where(diag, jnp.minimum(before + tot, CAP), 0.0).astype(bf16)
    sd = _iota((8, n_er), 0)
    sr = _iota((8, n_er), 1) & (ROWS - 1)
    start = _mm(_onehot(sr == 4 * sd), z0)
    end = _mm(_onehot(sr == 4 * sd + 3), z1)
    cnt = end - start
    off = _mm(cnt.astype(bf16), u_strict)
    tab_v[0:8, :] = start.astype(i32)
    tab_v[8:16, :] = cnt.astype(i32)
    tab_v[16:24, :] = off.astype(i32)
    tab_v[28:32, :] = jnp.zeros((4, 128), i32)
    tab_cp = pltpu.make_async_copy(tab_v, tab_s, misc_sem.at[1])
    tab_cp.start()

    base = pl.multiple_of((me >> 1) * 8, 8)
    idx8 = row_v[pl.ds(base, 8), :]
    ok8 = (row_v[pl.ds(ROWS + base, 8), :] > 0) & ((s8 >> 2) == (me & 1))
    e8 = _iota((N_EXP * 8, 128), 0) >> 3
    a = jnp.concatenate([jnp.where(ok8, idx8, -1)] * N_EXP, axis=0) == e8
    ab = _onehot(a)
    l256 = _onehot(_iota((256, 256), 1) < _iota((256, 256), 0))
    rank = _mm(ab, u_strict) + _mm(l256, _mm(ab, ones).astype(bf16))
    ra = jnp.where(a, rank, 0.0)
    slot8 = ra[0:8]
    for e in range(1, N_EXP):
        slot8 = slot8 + ra[e * 8:(e + 1) * 8]
    slot8 = jnp.where(ok8, slot8, -1.0)
    slot4 = jnp.where((me & 1) == 0, slot8[0:4], slot8[4:8])
    slot_t = jnp.transpose(jnp.concatenate([slot4, slot4], axis=0))
    lane512 = _iota((128, T_LOC), 1).astype(f32)
    for j in range(4):
        pmat[j * 128:(j + 1) * 128, :] = _onehot(slot_t[:, j:j + 1] == lane512)

    tab_cp.wait()

    def gather(e):
        def one(s, c):
            t = tab_s[24 + e // 2, (e % 2) * SLOTS + s]
            pltpu.make_async_copy(x_hbm.at[pl.ds(t, 1), :], xg.at[e, pl.ds(s, 1), :],
                                  g_sem.at[e]).start()
            return c
        lax.fori_loop(0, CAP, one, 0, unroll=True)

    def gather_wait(e):
        def one(s, c):
            pltpu.make_async_copy(x_hbm.at[pl.ds(0, 1), :], xg.at[e, pl.ds(0, 1), :],
                                  g_sem.at[e]).wait()
            return c
        lax.fori_loop(0, CAP, one, 0, unroll=True)

    def send(e, g):
        ge = me * E_LOC + e
        for k in range(N_DEV):
            d = (me + k) % N_DEV
            st, n, of = tab_s[d, ge], tab_s[8 + d, ge], tab_s[16 + d, ge]
            src = ybuf.at[g, pl.ds(e * SLOTS + st, n), :]
            dst = rbuf.at[g, pl.ds(of, n), :]

            @pl.when(n > 0)
            def _():
                if k == 0:
                    pltpu.make_async_copy(src, dst, recv_sem.at[g]).start()
                else:
                    pltpu.make_async_remote_copy(
                        src, dst, send_sem.at[g], recv_sem.at[g], device_id=(d,),
                        device_id_type=pl.DeviceIdType.MESH).start()

    last = N_EXP - 1
    n_recv = tab_s[16 + me, last] + tab_s[8 + me, last]

    def receive(g):
        @pl.when(n_recv > 0)
        def _():
            r = rbuf.at[g, pl.ds(0, n_recv), :]
            pltpu.make_async_copy(r, r, recv_sem.at[g]).wait()
        u = jnp.where(_iota((T_LOC, 128), 0) < n_recv, rbuf[g], jnp.uint32(0))
        lo_, hi_ = _unpack(u)
        obuf[:, g * 256:(g + 1) * 256] = _mm(pmat[...], jnp.concatenate([lo_, hi_], axis=1))

    def out_copy(g):
        cols = pl.ds(g * 256, 256)
        return pltpu.make_async_copy(obuf.at[:, cols], out_hbm.at[:, cols], out_sem.at[g])

    gather(0)
    n_steps = len(steps)
    for i, (e, g0, ng) in enumerate(steps):
        first = g0 == 0
        if first and e + 1 < E_LOC:
            gather(e + 1)
        w_copy(i).wait()
        if i + W_AHEAD < n_steps:
            w_copy(i + W_AHEAD).start()
        if i == n_steps - 1:
            for g in range(g0):
                out_copy(g).start()
        if first:
            gather_wait(e)
            xb[e] = xg[e].astype(bf16)
        y = _mm(xb[e], wbuf[e, :, g0 * 256:(g0 + ng) * 256].astype(bf16))
        for j in range(ng):
            ybuf[g0 + j, e * SLOTS:(e + 1) * SLOTS, :] = _pack(
                y[:, j * 256:j * 256 + 128], y[:, j * 256 + 128:(j + 1) * 256])
        if i == 0:
            pl.semaphore_wait(barrier, N_DEV - 1)
            for k in range(1, N_DEV):
                pl.semaphore_signal(done_sem, inc=1, device_id=((me + k) % N_DEV,),
                                    device_id_type=pl.DeviceIdType.MESH)
        for j in range(ng):
            send(e, g0 + j)
        if not first and e >= 2 and (e - 2) // 2 < g0 and e % 2 == 0:
            receive((e - 2) // 2)

    for g in range(PHASES[-1][0], NG):
        receive(g)
        out_copy(g).start()

    n_sent = jnp.int32(0)
    for e in range(E_LOC):
        for k in range(1, N_DEV):
            n_sent = n_sent + tab_s[8 + (me + k) % N_DEV, me * E_LOC + e]

    @pl.when(n_sent > 0)
    def _():
        for g in range(NG):
            r = ybuf.at[g, pl.ds(0, n_sent), :]
            pltpu.make_async_copy(r, r, send_sem.at[g]).wait()

    pl.semaphore_wait(done_sem, N_DEV - 1)
    for g in range(NG):
        out_copy(g).wait()


def pallas_dist_moe_cap_ep_outshard_n2048_d512_e8_h1024_kernel(x, router_W, route_idx, expert_W):
    del router_W
    idx = route_idx.astype(i32).reshape(ROWS, 128)
    any_spec = pl.BlockSpec(memory_space=pl.ANY)
    return pl.pallas_call(
        _body,
        out_shape=jax.ShapeDtypeStruct((T_LOC, H), f32),
        in_specs=[any_spec, any_spec, any_spec],
        out_specs=any_spec,
        scratch_shapes=[
            pltpu.VMEM((ROWS, 128), i32),
            pltpu.VMEM((2 * ROWS, 128), i32),
            pltpu.VMEM((32, 128), i32),
            pltpu.SMEM((32, 128), i32),
            pltpu.VMEM((E_LOC, SLOTS, D), f32),
            pltpu.VMEM((E_LOC, SLOTS, D), bf16),
            pltpu.VMEM((E_LOC, D, H), f32),
            pltpu.VMEM((NG, E_LOC * SLOTS, 128), u32),
            pltpu.VMEM((NG, T_LOC, 128), u32),
            pltpu.VMEM((T_LOC, T_LOC), bf16),
            pltpu.VMEM((T_LOC, H), f32),
            pltpu.SemaphoreType.DMA((2,)),
            pltpu.SemaphoreType.DMA((E_LOC * len(PHASES),)),
            pltpu.SemaphoreType.DMA((E_LOC,)),
            pltpu.SemaphoreType.DMA((NG,)),
            pltpu.SemaphoreType.DMA((NG,)),
            pltpu.SemaphoreType.DMA((NG,)),
            pltpu.SemaphoreType.REGULAR,
        ],
        compiler_params=pltpu.CompilerParams(collective_id=0, vmem_limit_bytes=64 * 1024 * 1024),
    )(x, idx, expert_W)
```

```python
import jax
import jax.numpy as jnp
from jax import lax
from jax.experimental import pallas as pl
from jax.experimental.pallas import tpu as pltpu

N_DEV = 4
N_TOK = 2048
D = 512
H = 1024
N_EXP = 32
E_LOC = N_EXP // N_DEV
CAP = 51
SLOTS = 64
T_LOC = N_TOK // N_DEV
ROWS = N_TOK // 128
NG = H // 256
PHASES = ((0, 3), (3, 1))
W_AHEAD = 2

f32, bf16, i32, u32 = jnp.float32, jnp.bfloat16, jnp.int32, jnp.uint32


def _iota(shape, dim):
    return lax.broadcasted_iota(i32, shape, dim)


def _mm(a, b):
    return jnp.dot(a, b, preferred_element_type=f32)


def _mm_nt(a, b):
    return lax.dot_general(a, b, (((1,), (1,)), ((), ())), preferred_element_type=f32)


def _onehot(cond):
    return jnp.where(cond, 1.0, 0.0).astype(bf16)


def _pack(lo, hi):
    lo = lax.bitcast_convert_type(lo.astype(bf16).astype(f32), u32)
    hi = lax.bitcast_convert_type(hi.astype(bf16).astype(f32), u32)
    return (lo >> 16) | (hi & jnp.uint32(0xFFFF0000))


def _unpack(u):
    lo = lax.bitcast_convert_type(u << 16, f32).astype(bf16)
    hi = lax.bitcast_convert_type(u & jnp.uint32(0xFFFF0000), f32).astype(bf16)
    return lo, hi


def _body(x_hbm, idx_hbm, w_hbm, obuf,
          idx_v, row_v, tab_v, tab_s, xg, xb, wbuf, ybuf, rbuf, pmat,
          misc_sem, w_sem, g_sem, send_sem, recv_sem, done_sem):
    me = lax.axis_index("i")

    steps = [(e, g0, ng) for (g0, ng) in PHASES for e in range(E_LOC)]

    def w_copy(i):
        e, g0, ng = steps[i]
        cols = pl.ds(g0 * 256, ng * 256)
        return pltpu.make_async_copy(w_hbm.at[e, :, cols], wbuf.at[e, :, cols], w_sem.at[i])

    idx_cp = pltpu.make_async_copy(idx_hbm, idx_v, misc_sem.at[0])
    idx_cp.start()
    for i in range(W_AHEAD):
        w_copy(i).start()

    barrier = pltpu.get_barrier_semaphore()
    for k in range(1, N_DEV):
        pl.semaphore_signal(barrier, inc=1, device_id=((me + k) % N_DEV,),
                            device_id_type=pl.DeviceIdType.MESH)

    xg[:, 48:SLOTS, :] = jnp.zeros((E_LOC, SLOTS - 48, D), f32)

    li = _iota((128, 128), 1)
    si = _iota((128, 128), 0)
    u_strict = _onehot(si < li)
    ones = jnp.ones((128, 128), bf16)
    n_er = N_EXP * ROWS
    rr = _iota((n_er, n_er), 0)
    cc = _iota((n_er, n_er), 1)
    l_blk = _onehot(((rr >> 4) == (cc >> 4)) & (cc < rr))

    idx_cp.wait()
    idx = idx_v[...] & (N_EXP - 1)

    er = _iota((n_er, 128), 0)
    m = jnp.concatenate([idx] * N_EXP, axis=0) == (er >> 4)
    mb = _onehot(m)
    within = _mm(mb, u_strict)
    tot = _mm(mb, ones)
    before = _mm(l_blk, tot.astype(bf16))
    pe = jnp.where(m, within + before, 0.0)
    pos = pe[0:ROWS]
    for e in range(1, N_EXP):
        pos = pos + pe[e * ROWS:(e + 1) * ROWS]
    pos = pos.astype(i32)
    ok = pos < CAP
    row_v[0:ROWS, :] = idx
    row_v[ROWS:2 * ROWS, :] = jnp.where(ok, 1, 0)

    key = jnp.where(ok & ((idx >> 3) == me), (idx & 7) * SLOTS + pos, -1)
    slot_i = _iota((E_LOC * SLOTS, 128), 0)
    acc = jnp.zeros((E_LOC * SLOTS, 128), i32)
    for r in range(ROWS):
        acc = jnp.where(slot_i == key[r:r + 1, :], r + 1, acc)
    s8 = _iota((8, 128), 0)
    l8 = _iota((8, 128), 1)
    hi = _mm_nt(jnp.ones((8, 128), bf16), acc.astype(f32).astype(bf16))
    lo = _mm_nt(l8.astype(f32).astype(bf16), _onehot(acc > 0))
    tok = jnp.maximum((hi.astype(i32) - 1) * 128 + lo.astype(i32), 0)
    for j in range(4):
        tab_v[24 + j:25 + j, :] = tok[0:1, j * 128:(j + 1) * 128]

    diag = _iota((n_er, 128), 1) == (er >> 4)
    z0 = jnp.where(diag, jnp.minimum(before, CAP), 0.0).astype(bf16)
    z1 = jnp.where(diag, jnp.minimum(before + tot, CAP), 0.0).astype(bf16)
    sd = _iota((8, n_er), 0)
    sr = _iota((8, n_er), 1) & (ROWS - 1)
    start = _mm(_onehot(sr == 4 * sd), z0)
    end = _mm(_onehot(sr == 4 * sd + 3), z1)
    cnt = end - start
    off = _mm(cnt.astype(bf16), u_strict)
    tab_v[0:8, :] = start.astype(i32)
    tab_v[8:16, :] = cnt.astype(i32)
    tab_v[16:24, :] = off.astype(i32)
    tab_v[28:32, :] = jnp.zeros((4, 128), i32)
    tab_cp = pltpu.make_async_copy(tab_v, tab_s, misc_sem.at[1])
    tab_cp.start()

    base = pl.multiple_of((me >> 1) * 8, 8)
    idx8 = row_v[pl.ds(base, 8), :]
    ok8 = (row_v[pl.ds(ROWS + base, 8), :] > 0) & ((s8 >> 2) == (me & 1))
    e8 = _iota((N_EXP * 8, 128), 0) >> 3
    a = jnp.concatenate([jnp.where(ok8, idx8, -1)] * N_EXP, axis=0) == e8
    ab = _onehot(a)
    l256 = _onehot(_iota((256, 256), 1) < _iota((256, 256), 0))
    rank = _mm(ab, u_strict) + _mm(l256, _mm(ab, ones).astype(bf16))
    ra = jnp.where(a, rank, 0.0)
    slot8 = ra[0:8]
    for e in range(1, N_EXP):
        slot8 = slot8 + ra[e * 8:(e + 1) * 8]
    slot8 = jnp.where(ok8, slot8, -1.0)
    slot4 = jnp.where((me & 1) == 0, slot8[0:4], slot8[4:8])
    slot_t = jnp.transpose(jnp.concatenate([slot4, slot4], axis=0))
    lane512 = _iota((128, T_LOC), 1).astype(f32)
    for j in range(4):
        pmat[j * 128:(j + 1) * 128, :] = _onehot(slot_t[:, j:j + 1] == lane512)

    tab_cp.wait()

    def gather(e):
        def one(s, c):
            t = tab_s[24 + e // 2, (e % 2) * SLOTS + s]
            pltpu.make_async_copy(x_hbm.at[pl.ds(t, 1), :], xg.at[e, pl.ds(s, 1), :],
                                  g_sem.at[e]).start()
            return c
        lax.fori_loop(0, CAP, one, 0, unroll=True)

    def gather_wait(e):
        def one(s, c):
            pltpu.make_async_copy(x_hbm.at[pl.ds(0, 1), :], xg.at[e, pl.ds(0, 1), :],
                                  g_sem.at[e]).wait()
            return c
        lax.fori_loop(0, CAP, one, 0, unroll=True)

    def send(e, g):
        ge = me * E_LOC + e
        for k in range(N_DEV):
            d = (me + k) % N_DEV
            st, n, of = tab_s[d, ge], tab_s[8 + d, ge], tab_s[16 + d, ge]
            src = ybuf.at[g, pl.ds(e * SLOTS + st, n), :]
            dst = rbuf.at[g, pl.ds(of, n), :]

            @pl.when(n > 0)
            def _():
                if k == 0:
                    pltpu.make_async_copy(src, dst, recv_sem.at[g]).start()
                else:
                    pltpu.make_async_remote_copy(
                        src, dst, send_sem.at[g], recv_sem.at[g], device_id=(d,),
                        device_id_type=pl.DeviceIdType.MESH).start()

    last = N_EXP - 1
    n_recv = tab_s[16 + me, last] + tab_s[8 + me, last]

    def receive(g):
        @pl.when(n_recv > 0)
        def _():
            r = rbuf.at[g, pl.ds(0, n_recv), :]
            pltpu.make_async_copy(r, r, recv_sem.at[g]).wait()
        u = jnp.where(_iota((T_LOC, 128), 0) < n_recv, rbuf[g], jnp.uint32(0))
        lo_, hi_ = _unpack(u)
        obuf[:, g * 256:(g + 1) * 256] = _mm(pmat[...], jnp.concatenate([lo_, hi_], axis=1))

    gather(0)
    received = 0
    for i, (e, g0, ng) in enumerate(steps):
        first = g0 == 0
        if first and e + 1 < E_LOC:
            gather(e + 1)
        w_copy(i).wait()
        if i + W_AHEAD < len(steps):
            w_copy(i + W_AHEAD).start()
        if first:
            gather_wait(e)
            xb[e] = xg[e].astype(bf16)
        y = _mm(xb[e], wbuf[e, :, g0 * 256:(g0 + ng) * 256].astype(bf16))
        for j in range(ng):
            ybuf[g0 + j, e * SLOTS:(e + 1) * SLOTS, :] = _pack(
                y[:, j * 256:j * 256 + 128], y[:, j * 256 + 128:(j + 1) * 256])
        if i == 0:
            pl.semaphore_wait(barrier, N_DEV - 1)
            for k in range(1, N_DEV):
                pl.semaphore_signal(done_sem, inc=1, device_id=((me + k) % N_DEV,),
                                    device_id_type=pl.DeviceIdType.MESH)
        for j in range(ng):
            send(e, g0 + j)
        if not first and e >= 2 and e % 2 == 0 and received < g0:
            receive(received)
            received += 1

    for g in range(received, NG):
        receive(g)

    n_sent = jnp.int32(0)
    for e in range(E_LOC):
        for k in range(1, N_DEV):
            n_sent = n_sent + tab_s[8 + (me + k) % N_DEV, me * E_LOC + e]

    @pl.when(n_sent > 0)
    def _():
        for g in range(NG):
            r = ybuf.at[g, pl.ds(0, n_sent), :]
            pltpu.make_async_copy(r, r, send_sem.at[g]).wait()

    pl.semaphore_wait(done_sem, N_DEV - 1)


def pallas_dist_moe_cap_ep_outshard_n2048_d512_e8_h1024_kernel(x, router_W, route_idx, expert_W):
    del router_W
    idx = route_idx.astype(i32).reshape(ROWS, 128)
    return pl.pallas_call(
        _body,
        out_shape=pltpu.VMEM((T_LOC, H), f32),
        in_specs=[pl.BlockSpec(memory_space=pl.ANY)] * 3,
        out_specs=pl.BlockSpec(memory_space=pltpu.VMEM),
        scratch_shapes=[
            pltpu.VMEM((ROWS, 128), i32),
            pltpu.VMEM((2 * ROWS, 128), i32),
            pltpu.VMEM((32, 128), i32),
            pltpu.SMEM((32, 128), i32),
            pltpu.VMEM((E_LOC, SLOTS, D), f32),
            pltpu.VMEM((E_LOC, SLOTS, D), bf16),
            pltpu.VMEM((E_LOC, D, H), f32),
            pltpu.VMEM((NG, E_LOC * SLOTS, 128), u32),
            pltpu.VMEM((NG, T_LOC, 128), u32),
            pltpu.VMEM((T_LOC, T_LOC), bf16),
            pltpu.SemaphoreType.DMA((2,)),
            pltpu.SemaphoreType.DMA((E_LOC * len(PHASES),)),
            pltpu.SemaphoreType.DMA((E_LOC,)),
            pltpu.SemaphoreType.DMA((NG,)),
            pltpu.SemaphoreType.DMA((NG,)),
            pltpu.SemaphoreType.REGULAR,
        ],
        compiler_params=pltpu.CompilerParams(collective_id=0, vmem_limit_bytes=64 * 1024 * 1024),
    )(x, idx, expert_W)
```
